```python
import numpy as np

kernel_name = "dist_sparse_attn_strided_kvseq_b1_sq256_skv4096_hq8_dh128"

def setup_inputs():
    x = np.random.randn(1, 256, 1024).astype(np.float32)
    Wq = np.random.randn(1024, 1024).astype(np.float32) * 0.02
    K_ext = np.random.randn(1, 16384, 8, 128).astype(np.float32)
    V_ext = np.random.randn(1, 16384, 8, 128).astype(np.float32)
    Wo = np.random.randn(1024, 1024).astype(np.float32) * 0.02
    return {"x": x, "Wq": Wq, "K_ext": K_ext, "V_ext": V_ext, "Wo": Wo}

def reference(x, Wq, K_ext, V_ext, Wo):
    B, Sq, Skv, Hq, Dh = 1, 256, 16384, 8, 128
    Q = (x @ Wq).reshape(B, Sq, Hq, Dh)
    qb = (np.arange(Sq) // 64)[:, None]
    kb = (np.arange(Skv) // 64)[None, :]
    mask = (qb == kb) | ((kb % 4) == (qb % 4))
    scores = np.einsum('bihd,bjhd->bhij', Q, K_ext).astype(np.float32) * 0.08838834764831843
    scores = np.where(mask[None, None, :, :], scores, -1e9)
    scores_max = scores.max(axis=-1, keepdims=True)
    w = np.exp(scores - scores_max)
    row_keep = mask.any(axis=1)
    w_sum = np.where(row_keep[None, None, :, None], w.sum(axis=-1, keepdims=True), 1.0)
    w = w / w_sum
    w = np.where(row_keep[None, None, :, None], w, 0.0)
    ctx = np.einsum('bhij,bjhd->bihd', w, V_ext).reshape(B, Sq, Hq * Dh)
    return ctx @ Wo
```

```python
import contextlib
import math

import jax
import jax.numpy as jnp
from jax import lax
from jax.experimental import pallas as pl
from jax.experimental.pallas import tpu as pltpu

N_DEV = 4
SQ, DM, HQ, DH = 256, 1024, 8, 128
QB = 64
NQB = SQ // QB
NKB = 16
NPIECE = HQ * NQB
Q_SCALE = 0.08838834764831843 * math.log2(math.e)
BF16, F32 = jnp.bfloat16, jnp.float32
MESH = pl.DeviceIdType.MESH


def make(shared_heads=3, wo_cols=128, lag=3, out_dtype=BF16, scopes=False,
         sem_checks=False, bounds_checks=False, ahead=13):
    own_heads = HQ - shared_heads
    own_rows = own_heads * DH
    share = shared_heads * DH // N_DEV
    n_wo = DM // wo_cols
    scope = jax.named_scope if scopes else (lambda name: contextlib.nullcontext())

    def body(x_hbm, wq_hbm, k_hbm, v_hbm, wo_hbm, out_ref,
             x_f32, wq_f32, wos_f32, wop_f32, kbuf, vbuf,
             x_all, q_all, wo_all, p_buf, part, stat, ctx, acc,
             w_sem, k_sem, v_sem, wo_sem, g_send, g_recv, p_send, s_send, p_recv, s_recv):
        me = lax.axis_index("i")
        right, diag, left = (lax.rem(me + d, N_DEV) for d in (1, 2, 3))

        x_copy = pltpu.make_async_copy(
            x_hbm.at[pl.ds(pl.multiple_of(me * QB, QB), QB)], x_f32, w_sem.at[0])
        wq_copy = pltpu.make_async_copy(
            wq_hbm.at[:, pl.ds(pl.multiple_of(me * 2 * DH, 2 * DH), 2 * DH)], wq_f32, w_sem.at[1])
        wos_copy = pltpu.make_async_copy(
            wo_hbm.at[pl.ds(pl.multiple_of(own_rows + me * share, 16), share)], wos_f32, w_sem.at[2])

        def kv_copy(src, dst, sem, n):
            return pltpu.make_async_copy(
                src.at[:, lax.rem(n, NQB), :, lax.div(n, NQB), :], dst.at[n], sem.at[n])

        def wo_copy(c):
            return pltpu.make_async_copy(
                wo_hbm.at[pl.ds(0, own_rows), pl.ds(c * wo_cols, wo_cols)], wop_f32.at[c], wo_sem.at[c])

        x_copy.start()
        barrier = pltpu.get_barrier_semaphore()
        for nbr in (left, right):
            pl.semaphore_signal(barrier, 1, device_id=(nbr,), device_id_type=MESH)
        wq_copy.start()
        wos_copy.start()

        def fetch(n):
            kv_copy(k_hbm, kbuf, k_sem, n).start()
            kv_copy(v_hbm, vbuf, v_sem, n).start()

        pl.loop(0, ahead)(fetch)

        def gather_copy(g, buf, owner, half, to, slot):
            return pltpu.make_async_remote_copy(
                buf.at[2 * owner + half], buf.at[2 * owner + half], g_send.at[g],
                g_recv.at[3 * g + slot], device_id=(to,), device_id_type=MESH)

        def gather_first(g, buf):
            gather_copy(g, buf, me, 0, right, 0).start()
            gather_copy(g, buf, me, 1, left, 1).start()

        def gather_second(g, buf):
            gather_copy(g, buf, me, 1, right, 2).start()
            gather_copy(g, buf, me, 0, left, 2).start()

        def gather_forward(g, buf):
            gather_copy(g, buf, left, 0, right, 0).wait_recv()
            gather_copy(g, buf, left, 0, right, 2).start()
            gather_copy(g, buf, right, 1, left, 1).wait_recv()
            gather_copy(g, buf, right, 1, left, 2).start()

        def gather_finish(g, buf):
            four = buf.at[pl.ds(0, 4)]
            pltpu.make_async_copy(four, four, g_recv.at[3 * g + 2]).wait()

        def gather_drain(g, buf):
            six = buf.at[pl.ds(0, 6)]
            pltpu.make_async_copy(six, six, g_send.at[g]).wait()

        with scope("x"):
            x_copy.wait()
            x_all[pl.ds(2 * me, 2)] = x_f32[...].astype(BF16).reshape(2, QB // 2, DM)
            pl.semaphore_wait(barrier, 2)
            gather_first(0, x_all)
            gather_second(0, x_all)
        with scope("xfwd"):
            gather_forward(0, x_all)
        with scope("wos"):
            wos_copy.wait()
            wo_all[pl.ds(2 * me, 2)] = wos_f32[...].astype(BF16).reshape(2, share // 2, DM)
            gather_first(2, wo_all)
            wq_copy.wait()
        with scope("xfin"):
            gather_finish(0, x_all)
        with scope("q"):
            q = jnp.dot(x_all[...].reshape(SQ, DM), wq_f32[...].astype(BF16),
                        preferred_element_type=F32) * Q_SCALE
            q_all[2 * me] = q[:, :DH].astype(BF16).reshape(NQB, QB, DH)
            q_all[2 * me + 1] = q[:, DH:].astype(BF16).reshape(NQB, QB, DH)
            gather_first(1, q_all)
            gather_second(1, q_all)
        with scope("qfwd"):
            gather_forward(1, q_all)
            gather_second(2, wo_all)
            gather_forward(2, wo_all)
        with scope("qfin"):
            gather_finish(1, q_all)

        row = lax.broadcasted_iota(jnp.int32, (QB, DH), 0)
        lane = lax.broadcasted_iota(jnp.int32, (QB, DH), 1)

        def broadcast(buf, n, send, recv):
            for d, to in ((2, diag), (1, right), (3, left)):
                pltpu.make_async_remote_copy(
                    buf.at[n, pl.ds(0, 1)], buf.at[n, pl.ds(d, 1)], send, recv.at[n],
                    device_id=(to,), device_id_type=MESH).start()

        def wait_others(buf, n, recv):
            three = buf.at[n, pl.ds(1, 3)]
            pltpu.make_async_copy(three, three, recv.at[n]).wait()

        def scores(n):
            kv_copy(k_hbm, kbuf, k_sem, n).wait()
            k = kbuf[n].reshape(NKB * QB, DH).astype(BF16)
            s = lax.dot_general(q_all[lax.div(n, NQB), lax.rem(n, NQB)], k,
                                (((1,), (1,)), ((), ())), preferred_element_type=F32)
            m = jnp.max(s, axis=1, keepdims=True)
            p = jnp.exp2(s - m)
            l = jnp.sum(p, axis=1, keepdims=True)
            p_buf[...] = p.astype(BF16)
            packed = jnp.where(lane == row, m, jnp.where(lane == row + QB, l, 0.0))
            stat[n, 0] = jnp.sum(packed, axis=0, keepdims=True)
            broadcast(stat, n, s_send, s_recv)

        def values(n):
            kv_copy(v_hbm, vbuf, v_sem, n).wait()
            v = vbuf[n].reshape(NKB * QB, DH).astype(BF16)
            part[n, 0] = jnp.dot(p_buf[...], v, preferred_element_type=F32).astype(BF16)
            broadcast(part, n, p_send, p_recv)

        def weights(n):
            wait_others(stat, n, s_recv)
            st = [stat[n, d] for d in range(N_DEV)]
            top = jnp.maximum(jnp.maximum(st[0], st[1]), jnp.maximum(st[2], st[3]))
            e = [jnp.exp2(t - top) for t in st]
            total = sum(ei * pltpu.roll(t, QB, 1) for ei, t in zip(e, st))
            low = lane[:1] < QB
            inv = 1.0 / jnp.where(low, total, 1.0)
            w = []
            for a in (0, 2):
                pair = jnp.where(low, e[a] * inv, pltpu.roll(e[a + 1] * inv, QB, 1))
                cols = jnp.broadcast_to(pair, (DH, DH)).T
                w += [cols[:QB], cols[QB:]]
            return w

        def combine(n, w):
            wait_others(part, n, p_recv)
            return sum(w[d] * part[n, d].astype(F32) for d in range(N_DEV)).astype(BF16)

        def head_ctx(h):
            return ctx[pl.ds(NQB * h, NQB)].reshape(SQ, DH)

        with scope("loop"):
            @pl.loop(0, NPIECE)
            def _(n):
                @pl.when(n + ahead < NPIECE)
                def _():
                    fetch(n + ahead)

                @pl.when(n == NPIECE - 4)
                def _():
                    for c in range(n_wo):
                        wo_copy(c).start()

                with scope("s"):
                    scores(n)

                with scope("c"):
                    @pl.when(n >= lag)
                    def _():
                        ctx[n - lag] = combine(n - lag, weights(n - lag))

                with scope("v"):
                    values(n)

        with scope("shared"):
            gather_finish(2, wo_all)
            wo_shared = wo_all[...].reshape(shared_heads * DH, DM)
            early = jnp.concatenate([head_ctx(h) for h in range(own_heads, HQ - 1)], axis=1)
            acc[...] = jnp.dot(early, wo_shared[:-DH], preferred_element_type=F32)

        for c in range(n_wo):
            with scope("wo%d" % c):
                wo_copy(c).wait()
                lhs = jnp.concatenate([head_ctx(h) for h in range(own_heads)], axis=1)
                cols = pl.ds(c * wo_cols, wo_cols)
                acc[:, cols] += jnp.dot(lhs, wop_f32[c].astype(BF16), preferred_element_type=F32)

        with scope("late"):
            for n in range(NPIECE - lag, NPIECE - 1):
                ctx[n] = combine(n, weights(n))
            wo_last = wo_all[...].reshape(shared_heads * DH, DM)[-DH:]
            rows = pl.ds(0, SQ - QB)
            lhs = ctx[pl.ds(NPIECE - NQB, NQB - 1)].reshape(SQ - QB, DH)
            out_ref[rows] = (acc[rows] + jnp.dot(lhs, wo_last, preferred_element_type=F32)).astype(out_dtype)

        with scope("drain"):
            for g, buf in enumerate((x_all, q_all, wo_all)):
                gather_drain(g, buf)
            for buf, sem in ((stat, s_send), (part, p_send)):
                sent = buf.at[:, pl.ds(1, 3)]
                pltpu.make_async_copy(sent, sent, sem).wait()

        with scope("lastw"):
            w = weights(NPIECE - 1)
        with scope("last"):
            lhs = combine(NPIECE - 1, w)
            wo_last = wo_all[...].reshape(shared_heads * DH, DM)[-DH:]
            rows = pl.ds(SQ - QB, QB)
            out_ref[rows] = (acc[rows] + jnp.dot(lhs, wo_last, preferred_element_type=F32)).astype(out_dtype)

    dma = pltpu.SemaphoreType.DMA

    def fn(x, Wq, K_ext, V_ext, Wo):
        kv_shape = (NKB, NQB, QB, HQ, DH)
        out = pl.pallas_call(
            body,
            out_shape=jax.ShapeDtypeStruct((SQ, DM), out_dtype),
            in_specs=[pl.BlockSpec(memory_space=pl.ANY)] * 5,
            out_specs=pl.BlockSpec(memory_space=pltpu.VMEM),
            scratch_shapes=[
                pltpu.VMEM((QB, DM), F32),
                pltpu.VMEM((DM, 2 * DH), F32),
                pltpu.VMEM((share, DM), F32),
                pltpu.VMEM((n_wo, own_rows, wo_cols), F32),
                pltpu.VMEM((NPIECE, NKB, QB, DH), F32),
                pltpu.VMEM((NPIECE, NKB, QB, DH), F32),
                pltpu.VMEM((2 * N_DEV, QB // 2, DM), BF16),
                pltpu.VMEM((HQ, NQB, QB, DH), BF16),
                pltpu.VMEM((2 * N_DEV, share // 2, DM), BF16),
                pltpu.VMEM((QB, NKB * QB), BF16),
                pltpu.VMEM((NPIECE, N_DEV, QB, DH), BF16),
                pltpu.VMEM((NPIECE, N_DEV, 1, DH), F32),
                pltpu.VMEM((NPIECE, QB, DH), BF16),
                pltpu.VMEM((SQ, DM), F32),
                dma((3,)), dma((NPIECE,)), dma((NPIECE,)), dma((n_wo,)),
                dma((3,)), dma((9,)), dma, dma, dma((NPIECE,)), dma((NPIECE,)),
            ],
            compiler_params=pltpu.CompilerParams(
                collective_id=0, vmem_limit_bytes=100 << 20,
                disable_semaphore_checks=not sem_checks,
                disable_bounds_checks=not bounds_checks),
        )(x.reshape(SQ, DM), Wq, K_ext.reshape(kv_shape), V_ext.reshape(kv_shape), Wo)
        return out.reshape(1, SQ, DM)

    return fn


def pallas_dist_sparse_attn_strided_kvseq_b1_sq256_skv4096_hq8_dh128_kernel(x, Wq, K_ext, V_ext, Wo):
    return make()(x, Wq, K_ext, V_ext, Wo)
```

```python
import math

import jax
import jax.numpy as jnp
from jax import lax
from jax.experimental import pallas as pl
from jax.experimental.pallas import tpu as pltpu

N_DEV = 4
SQ, DM, HQ, DH = 256, 1024, 8, 128
QB = 64
NQB = SQ // QB
NKB = 16
NPIECE = HQ * NQB
LAST = NPIECE - 1
EARLY_HEADS = 4
N_EARLY = EARLY_HEADS * NQB
LAG = 2
WQ_PARTS = 8
WO_COLS = 512
COL_PARTS = DM // WO_COLS
N_CHUNK = EARLY_HEADS * COL_PARTS
LEAD_ROWS = 16
Q_SCALE = 0.08838834764831843 * math.log2(math.e)
BF16, F32 = jnp.bfloat16, jnp.float32
MESH = pl.DeviceIdType.MESH

WO_SHARE = (176, 144, 0, 192)
WO_START = tuple(sum(WO_SHARE[:c]) for c in range(N_DEV))
WO_SPLIT = tuple((rows + 31) // 32 * 16 for rows in WO_SHARE)
WO_OWNERS = tuple(c for c in range(N_DEV) if WO_SHARE[c])
HOP_ORDER = ((2, 1, 3), (3, 2, 1), (2, 1, 3), (1, 2, 3))

GATHER_X, GATHER_Q, GATHER_WO = range(3)
N_SLOT = 6
SLOT_HALF = (0, 1, 1, 0, 0, 1)
OWNER_FROM_SENDER = (0, 0, 0, 0, 3, 1)
OWNER_FROM_RECEIVER = (3, 1, 3, 1, 2, 2)

FINISH = (
    (0, None, 29), (1, 29, None), (2, None, None), (3, None, 30), (4, None, None),
    (5, 30, None), (6, None, None), (7, None, 31), (None, 31, None),
)
FINISH_CHIP_3 = (
    (0, None, 29), (1, 29, 30), (2, 30, None), (3, None, None), (4, None, 31),
    (5, 31, None), (6, None, None), (7, None, None),
)


def _body(x_hbm, wq_hbm, k_hbm, v_hbm, wo_hbm, out_ref,
          x_mine, wq_mine, wo_mine, wo_early, k_buf, v_buf,
          x_all, q_all, wo_late, p_buf, carry, w_buf, part, stat, ctx, acc,
          w_sem, k_sem, v_sem, wo_sem, g_send, g_recv, c_send, c_recv,
          p_send, s_send, p_recv, s_recv):
    def k_copy(n):
        h, j = n >> 2, n & 3
        return pltpu.make_async_copy(k_hbm.at[:, j, :, h], k_buf.at[h, :, j], k_sem.at[n])

    def v_copy(n):
        h, j = n >> 2, n & 3
        return pltpu.make_async_copy(v_hbm.at[:, j, :, h], v_buf.at[h, :, j], v_sem.at[n])

    def last_v_copy(i):
        blocks = pl.ds(i * (NKB // 2), NKB // 2)
        return pltpu.make_async_copy(
            v_hbm.at[blocks, NQB - 1, :, HQ - 1], v_buf.at[HQ - 1, blocks, NQB - 1],
            v_sem.at[LAST + i])

    def head_copies(h):
        return (pltpu.make_async_copy(k_hbm.at[:, :, :, h], k_buf.at[h], k_sem.at[NQB * h]),
                pltpu.make_async_copy(v_hbm.at[:, :, :, h], v_buf.at[h], v_sem.at[NQB * h]))

    def fetch(n):
        k_copy(n).start()
        v_copy(n).start()

    k_copy(0).start()

    me = lax.axis_index("i")

    def ahead(d):
        return (me + d) & (N_DEV - 1)

    def on_chip(c):
        return pl.when(me == c % N_DEV)

    def remote(src, dst, send_sem, recv_sem, d):
        return pltpu.make_async_remote_copy(
            src, dst, send_sem, recv_sem, device_id=(ahead(d),), device_id_type=MESH)

    def wait_filled(ref, sem):
        pltpu.make_async_copy(ref, ref, sem).wait()

    x_copy = pltpu.make_async_copy(
        x_hbm.at[pl.ds(pl.multiple_of(me * QB, QB), QB)], x_mine, w_sem.at[0])

    def wq_copy(i):
        rows = pl.ds(i * (DM // WQ_PARTS), DM // WQ_PARTS)
        cols = pl.ds(pl.multiple_of(me * 2 * DH, 2 * DH), 2 * DH)
        return pltpu.make_async_copy(wq_hbm.at[rows, cols], wq_mine.at[rows], w_sem.at[1])

    def wo_mine_copy(c):
        return pltpu.make_async_copy(
            wo_hbm.at[pl.ds(EARLY_HEADS * DH + WO_START[c], WO_SHARE[c])],
            wo_mine.at[pl.ds(0, WO_SHARE[c])], w_sem.at[2])

    def wo_early_copy(c):
        h, i = divmod(c, COL_PARTS)
        return pltpu.make_async_copy(
            wo_hbm.at[pl.ds(h * DH, DH), pl.ds(i * WO_COLS, WO_COLS)],
            wo_early.at[c], wo_sem.at[c])

    def fetch_wo_early():
        for c in range(N_CHUNK):
            wo_early_copy(c).start()

    barrier = pltpu.get_barrier_semaphore()
    for d in range(1, N_DEV):
        pl.semaphore_signal(barrier, 1, device_id=(ahead(d),), device_id_type=MESH)

    wq_copy(0).start()
    x_copy.start()
    wq_copy(1).start()
    for c in WO_OWNERS:
        on_chip(c)(lambda c=c: wo_mine_copy(c).start())
    v_copy(0).start()
    for n in range(1, NQB):
        wq_copy(2 * n).start()
        k_copy(n).start()
        wq_copy(2 * n + 1).start()
        v_copy(n).start()
    for h in range(1, EARLY_HEADS):
        for copy in head_copies(h):
            copy.start()

    def gather_copy(g, slot, owner):
        half = SLOT_HALF[slot]
        if g == GATHER_WO:
            rows = WO_SHARE[owner] - WO_SPLIT[owner] if half else WO_SPLIT[owner]
            ref = wo_late.at[pl.ds(WO_START[owner] + half * WO_SPLIT[owner], rows)]
        else:
            ref = (x_all, q_all)[g].at[2 * owner + half]
        i = N_SLOT * g + slot
        return remote(ref, ref, g_send.at[i], g_recv.at[i], 3 if slot % 2 else 1)

    def each_gather_copy(g, slots, offsets, action):
        for slot in slots:
            if g == GATHER_WO:
                for owner in WO_OWNERS:
                    on_chip(owner - offsets[slot])(
                        lambda slot=slot, owner=owner: action(gather_copy(g, slot, owner)))
            else:
                action(gather_copy(g, slot, ahead(offsets[slot])))

    def send(g, slots):
        each_gather_copy(g, slots, OWNER_FROM_SENDER, lambda copy: copy.start())

    def receive(g, slots):
        each_gather_copy(g, slots, OWNER_FROM_RECEIVER, lambda copy: copy.wait_recv())

    def relay(g):
        for slot in (0, 1):
            receive(g, (slot,))
            send(g, (slot + 4,))

    acc[...] = jnp.zeros_like(acc)
    x_copy.wait()
    x_all[pl.ds(2 * me, 2)] = x_mine[...].astype(BF16).reshape(2, QB // 2, DM)
    pl.semaphore_wait(barrier, N_DEV - 1)
    send(GATHER_X, (0, 1, 2, 3))
    relay(GATHER_X)

    for c in WO_OWNERS:
        @on_chip(c)
        def _(c=c):
            wo_mine_copy(c).wait()
            wo_late[pl.ds(WO_START[c], WO_SHARE[c])] = (
                wo_mine[pl.ds(0, WO_SHARE[c])].astype(BF16))

    send(GATHER_WO, (0, 1))
    wait_filled(wq_mine, w_sem.at[1])
    receive(GATHER_X, (2, 3, 4, 5))
    q = jnp.dot(x_all[...].reshape(SQ, DM), wq_mine[...].astype(BF16),
                preferred_element_type=F32) * Q_SCALE
    for i in (0, 1):
        q_all[2 * me + i] = q[:, i * DH:(i + 1) * DH].astype(BF16).reshape(NQB, QB, DH)
    send(GATHER_Q, (0, 1, 2, 3))
    relay(GATHER_Q)
    send(GATHER_WO, (2, 3))
    relay(GATHER_WO)
    receive(GATHER_Q, (2, 3, 4, 5))

    row = lax.broadcasted_iota(jnp.int32, (QB, DH), 0)
    lane = lax.broadcasted_iota(jnp.int32, (QB, DH), 1)
    on_diagonal = (lane & (QB - 1)) == row

    hops = []
    for i in range(N_DEV - 1):
        d = jnp.int32(HOP_ORDER[0][i])
        for c in range(1, N_DEV):
            d = jnp.where(me == c, HOP_ORDER[c][i], d)
        hops.append(d)

    def send_stat(n, d):
        remote(stat.at[n, 0], stat.at[n, d], s_send, s_recv.at[n], d).start()

    def send_part(n, d):
        remote(part.at[n, 0], part.at[n, d], p_send, p_recv.at[n], d).start()

    def wait_stats(n):
        wait_filled(stat.at[n, pl.ds(1, N_DEV - 1)], s_recv.at[n])

    def wait_parts(n):
        wait_filled(part.at[n, pl.ds(1, N_DEV - 1)], p_recv.at[n])

    def probabilities(n):
        k = k_buf[n >> 2, :, n & 3].reshape(NKB * QB, DH).astype(BF16)
        s = lax.dot_general(q_all[n >> 2, n & 3], k, (((1,), (1,)), ((), ())),
                            preferred_element_type=F32)
        row_max = jnp.max(s, axis=1, keepdims=True)
        p = jnp.exp2(s - row_max)
        p_buf[...] = p.astype(BF16)
        lane_sums = p[:, :DH]
        for i in range(1, NKB * QB // DH):
            lane_sums = lane_sums + p[:, i * DH:(i + 1) * DH]
        return row_max, lane_sums

    def store_stats(n, row_max, lane_sums):
        for i, column in enumerate((row_max, jnp.sum(lane_sums, axis=1, keepdims=True))):
            stat[n, 0, pl.ds(i, 1)] = jnp.sum(
                jnp.where(on_diagonal, column, 0.0), axis=0, keepdims=True)

    def weighted_values(n, start=0, size=NKB):
        v = v_buf[n >> 2, pl.ds(start, size), n & 3].reshape(size * QB, DH).astype(BF16)
        return jnp.dot(p_buf[:, pl.ds(start * QB, size * QB)], v, preferred_element_type=F32)

    def merge_weights(n):
        m = [stat[n, d, pl.ds(0, 1)] for d in range(N_DEV)]
        top = jnp.maximum(jnp.maximum(m[0], m[1]), jnp.maximum(m[2], m[3]))
        e = [jnp.exp2(local - top) for local in m]
        inv = 1.0 / sum(e[d] * stat[n, d, pl.ds(1, 1)] for d in range(N_DEV))
        for a in (0, 1):
            pair = jnp.where(lane[:1] < QB, e[2 * a], e[2 * a + 1]) * inv
            w_buf[n & 1, pl.ds(a * DH, DH)] = jnp.broadcast_to(pair, (DH, DH)).T

    def merged(n):
        t = [w_buf[n & 1, pl.ds(d * QB, QB)] * part[n, d].astype(F32) for d in range(N_DEV)]
        return ((t[0] + t[1]) + (t[2] + t[3])).astype(BF16)

    for n in range(NQB):
        k_copy(n).wait()
        v_copy(n).wait()
    pl.loop(N_EARLY, NPIECE - NQB)(fetch)

    @pl.loop(0, N_EARLY)
    def _(n):
        @pl.when((n > 0) & ((n & 3) == 0))
        def _():
            for copy in head_copies(n >> 2):
                copy.wait()

        store_stats(n, *probabilities(n))
        part[n, 0] = weighted_values(n).astype(BF16)
        to_owner = (n + N_DEV - me) & (N_DEV - 1)

        @pl.when(to_owner != 0)
        def _():
            send_stat(n, to_owner)
            send_part(n, to_owner)

    def late_piece(n, weights_for=None):
        k_copy(n).wait()
        store_stats(n, *probabilities(n))
        for d in hops:
            send_stat(n, d)
        if weights_for is not None:
            wait_stats(weights_for)
        v_copy(n).wait()
        if weights_for is not None:
            merge_weights(weights_for)
        part[n, 0] = weighted_values(n).astype(BF16)
        for d in hops:
            send_part(n, d)

    pl.loop(N_EARLY, N_EARLY + LAG)(late_piece)

    @pl.loop(0, EARLY_HEADS)
    def _(h):
        n = h * NQB + me
        wait_stats(n)
        wait_parts(n)
        merge_weights(n)
        ctx[me, h] = merged(n)

    def ctx_copy(d, owner):
        return remote(ctx.at[owner], ctx.at[owner], c_send.at[d - 1], c_recv.at[d - 1], d)

    for d in (2, 1, 3):
        ctx_copy(d, me).start()
    receive(GATHER_WO, (2, 3, 4, 5))

    @pl.loop(N_EARLY + LAG, LAST)
    def _(n):
        @pl.when(n == NPIECE - 2 * NQB)
        def _():
            pl.loop(NPIECE - NQB, LAST)(fetch)
            k_copy(LAST).start()
            last_v_copy(0).start()
            last_v_copy(1).start()
            pl.when(me != 2)(fetch_wo_early)

        done = n - LAG
        late_piece(n, done)
        wait_parts(done)
        wo = wo_late[pl.ds(pl.multiple_of(((done >> 2) - EARLY_HEADS) * DH, DH), DH)]
        rows = pl.ds(pl.multiple_of((done & 3) * QB, QB), QB)
        acc[rows] += jnp.dot(merged(done), wo, preferred_element_type=F32)

    for d in range(1, N_DEV):
        ctx_copy(d, ahead(N_DEV - d)).wait_recv()
        ctx_copy(d, me).wait_send()
    for g in (GATHER_X, GATHER_Q, GATHER_WO):
        each_gather_copy(g, range(N_SLOT), OWNER_FROM_SENDER, lambda copy: copy.wait_send())

    k_copy(LAST).wait()
    row_max, lane_sums = probabilities(LAST)
    carry[0] = jnp.broadcast_to(row_max, (QB, DH))
    carry[1] = lane_sums
    last_v_copy(0).wait()
    carry[2] = weighted_values(LAST, 0, NKB // 2)
    store_stats(LAST, carry[0], carry[1])
    for d in hops:
        send_stat(LAST, d)
    last_v_copy(1).wait()
    local = carry[2] + weighted_values(LAST, NKB // 2, NKB // 2)
    for start, size in ((0, LEAD_ROWS), (LEAD_ROWS, QB - LEAD_ROWS)):
        rows = pl.ds(start, size)
        part[LAST, 0, rows] = local[start:start + size].astype(BF16)
        remote(part.at[LAST, 0, rows], part.at[LAST, hops[0], rows],
               p_send, p_recv.at[LAST], hops[0]).start()
    for d in hops[1:]:
        send_part(LAST, d)
    on_chip(2)(fetch_wo_early)

    def finish(steps):
        for i, (chunk, piece, weights_for) in enumerate(steps):
            if i == len(steps) - 1:
                sent = (pl.ds(0, EARLY_HEADS + NPIECE - N_EARLY), pl.ds(1, N_DEV - 1))
                wait_filled(stat.at[sent], s_send)
                wait_filled(part.at[sent], p_send)
            if chunk is not None:
                wo_early_copy(chunk).wait()
            if piece is not None:
                wait_parts(piece)
            if weights_for is not None:
                wait_stats(weights_for)

            if chunk is not None:
                h, c = divmod(chunk, COL_PARTS)
                cols = pl.ds(c * WO_COLS, WO_COLS)
                total = acc[:, cols] + jnp.dot(
                    ctx[:, h].reshape(SQ, DH), wo_early[chunk].astype(BF16),
                    preferred_element_type=F32)
                acc[:, cols] = total
                if h == EARLY_HEADS - 1:
                    out_ref[:, cols] = total.astype(out_ref.dtype)
            if piece is not None:
                h, j = divmod(piece, NQB)
                rows = pl.ds(j * QB, QB)
                total = acc[rows] + jnp.dot(
                    merged(piece), wo_late[pl.ds((h - EARLY_HEADS) * DH, DH)],
                    preferred_element_type=F32)
                if chunk is None:
                    out_ref[rows] = total.astype(out_ref.dtype)
                else:
                    acc[rows] = total
            if weights_for is not None:
                merge_weights(weights_for)

    pl.when(me == 3)(lambda: finish(FINISH_CHIP_3))
    pl.when(me != 3)(lambda: finish(FINISH))


def pallas_dist_sparse_attn_strided_kvseq_b1_sq256_skv4096_hq8_dh128_kernel(
    x: jax.Array,
    Wq: jax.Array,
    K_ext: jax.Array,
    V_ext: jax.Array,
    Wo: jax.Array,
):
    dma = pltpu.SemaphoreType.DMA
    kv_shape = (NKB, NQB, QB, HQ, DH)
    out = pl.pallas_call(
        _body,
        out_shape=jax.ShapeDtypeStruct((SQ, DM), BF16),
        in_specs=[pl.BlockSpec(memory_space=pl.ANY)] * 5,
        out_specs=pl.BlockSpec(memory_space=pltpu.VMEM),
        scratch_shapes=[
            pltpu.VMEM((QB, DM), F32),
            pltpu.VMEM((DM, 2 * DH), F32),
            pltpu.VMEM((max(WO_SHARE), DM), F32),
            pltpu.VMEM((N_CHUNK, DH, WO_COLS), F32),
            pltpu.VMEM((HQ, NKB, NQB, QB, DH), F32),
            pltpu.VMEM((HQ, NKB, NQB, QB, DH), F32),
            pltpu.VMEM((2 * N_DEV, QB // 2, DM), BF16),
            pltpu.VMEM((HQ, NQB, QB, DH), BF16),
            pltpu.VMEM((DM - EARLY_HEADS * DH, DM), BF16),
            pltpu.VMEM((QB, NKB * QB), BF16),
            pltpu.VMEM((3, QB, DH), F32),
            pltpu.VMEM((2, N_DEV * QB, DH), F32),
            pltpu.VMEM((NPIECE, N_DEV, QB, DH), BF16),
            pltpu.VMEM((NPIECE, N_DEV, 2, DH), F32),
            pltpu.VMEM((NQB, EARLY_HEADS, QB, DH), BF16),
            pltpu.VMEM((SQ, DM), F32),
            dma((3,)), dma((NPIECE,)), dma((NPIECE + 1,)), dma((N_CHUNK,)),
            dma((3 * N_SLOT,)), dma((3 * N_SLOT,)), dma((N_DEV - 1,)), dma((N_DEV - 1,)),
            dma, dma, dma((NPIECE,)), dma((NPIECE,)),
        ],
        compiler_params=pltpu.CompilerParams(
            collective_id=0,
            vmem_limit_bytes=64 << 20,
            disable_bounds_checks=True,
            disable_semaphore_checks=True,
        ),
    )(x.reshape(SQ, DM), Wq, K_ext.reshape(kv_shape), V_ext.reshape(kv_shape), Wo)
    return out.reshape(1, SQ, DM)
```

```python
import math

import jax
import jax.numpy as jnp
from jax import lax
from jax.experimental import pallas as pl
from jax.experimental.pallas import tpu as pltpu

N_DEV = 4
SQ, DM, HQ, DH = 256, 1024, 8, 128
QB = 64
NQB = SQ // QB
NKB = 16
NPIECE = HQ * NQB
LAST = NPIECE - 1
EARLY_HEADS = 4
N_EARLY = EARLY_HEADS * NQB
LAG = 2
WQ_PARTS = 16
WO_COLS = 512
COL_PARTS = DM // WO_COLS
N_CHUNK = EARLY_HEADS * COL_PARTS
LEAD_ROWS = 16
Q_SCALE = 0.08838834764831843 * math.log2(math.e)
BF16, F32 = jnp.bfloat16, jnp.float32
MESH = pl.DeviceIdType.MESH

WO_SHARE = (160, 144, 0, 208)
WO_START = tuple(sum(WO_SHARE[:c]) for c in range(N_DEV))
WO_SPLIT = tuple((rows + 31) // 32 * 16 for rows in WO_SHARE)
WO_OWNERS = tuple(c for c in range(N_DEV) if WO_SHARE[c])
HOP_ORDER = ((2, 1, 3), (3, 2, 1), (2, 1, 3), (1, 2, 3))

GATHER_X, GATHER_Q, GATHER_WO = range(3)
N_SLOT = 6
SLOT_HALF = (0, 1, 1, 0, 0, 1)
OWNER_FROM_SENDER = (0, 0, 0, 0, 3, 1)
OWNER_FROM_RECEIVER = (3, 1, 3, 1, 2, 2)

FINISH = (
    (0, None, 29), (1, 29, None), (2, None, None), (3, None, 30), (4, None, None),
    (5, 30, None), (6, None, None), (7, None, 31), (None, 31, None),
)
FINISH_CHIP_3 = (
    (0, None, 29), (1, 29, 30), (2, 30, None), (3, None, None), (4, None, 31),
    (5, 31, None), (6, None, None), (7, None, None),
)


def _body(x_hbm, wq_hbm, k_hbm, v_hbm, wo_hbm, out_ref,
          x_mine, wq_mine, wo_mine, wo_early, k_buf, v_buf,
          x_all, q_all, wo_late, p_buf, carry, w_buf, part, stat, ctx, acc,
          w_sem, k_sem, v_sem, wo_sem, g_send, g_recv, c_send, c_recv,
          p_send, s_send, p_recv, s_recv):
    def k_copy(n):
        h, j = n >> 2, n & 3
        return pltpu.make_async_copy(k_hbm.at[:, j, :, h], k_buf.at[h, :, j], k_sem.at[n])

    def v_copy(n):
        h, j = n >> 2, n & 3
        return pltpu.make_async_copy(v_hbm.at[:, j, :, h], v_buf.at[h, :, j], v_sem.at[n])

    def last_v_copy(i):
        blocks = pl.ds(i * (NKB // 2), NKB // 2)
        return pltpu.make_async_copy(
            v_hbm.at[blocks, NQB - 1, :, HQ - 1], v_buf.at[HQ - 1, blocks, NQB - 1],
            v_sem.at[LAST + i])

    def head_copies(h):
        return (pltpu.make_async_copy(k_hbm.at[:, :, :, h], k_buf.at[h], k_sem.at[NQB * h]),
                pltpu.make_async_copy(v_hbm.at[:, :, :, h], v_buf.at[h], v_sem.at[NQB * h]))

    def first_head_copy(src, dst, sem, i):
        size = 2 * NKB // WQ_PARTS
        blocks = pl.ds(i * size, size)
        return pltpu.make_async_copy(src.at[blocks, :, :, 0], dst.at[0, blocks], sem.at[0])

    def fetch(n):
        k_copy(n).start()
        v_copy(n).start()

    first_head_copy(k_hbm, k_buf, k_sem, 0).start()

    me = lax.axis_index("i")

    def ahead(d):
        return (me + d) & (N_DEV - 1)

    def on_chip(c):
        return pl.when(me == c % N_DEV)

    def remote(src, dst, send_sem, recv_sem, d):
        return pltpu.make_async_remote_copy(
            src, dst, send_sem, recv_sem, device_id=(ahead(d),), device_id_type=MESH)

    def wait_filled(ref, sem):
        pltpu.make_async_copy(ref, ref, sem).wait()

    x_copy = pltpu.make_async_copy(
        x_hbm.at[pl.ds(pl.multiple_of(me * QB, QB), QB)], x_mine, w_sem.at[0])

    def wq_copy(i):
        size = DM // WQ_PARTS
        rows = pl.ds(i * size if isinstance(i, int) else pl.multiple_of(i * size, size), size)
        cols = pl.ds(pl.multiple_of(me * 2 * DH, 2 * DH), 2 * DH)
        return pltpu.make_async_copy(wq_hbm.at[rows, cols], wq_mine.at[rows], w_sem.at[1])

    def wo_mine_copy(c):
        return pltpu.make_async_copy(
            wo_hbm.at[pl.ds(EARLY_HEADS * DH + WO_START[c], WO_SHARE[c])],
            wo_mine.at[pl.ds(0, WO_SHARE[c])], w_sem.at[2])

    def wo_early_copy(c):
        h, i = divmod(c, COL_PARTS)
        return pltpu.make_async_copy(
            wo_hbm.at[pl.ds(h * DH, DH), pl.ds(i * WO_COLS, WO_COLS)],
            wo_early.at[c], wo_sem.at[c])

    def fetch_wo_early():
        for c in range(N_CHUNK):
            wo_early_copy(c).start()

    barrier = pltpu.get_barrier_semaphore()
    for d in range(1, N_DEV):
        pl.semaphore_signal(barrier, 1, device_id=(ahead(d),), device_id_type=MESH)

    wq_copy(0).start()
    x_copy.start()
    for c in WO_OWNERS:
        on_chip(c)(lambda c=c: wo_mine_copy(c).start())

    @pl.loop(1, WQ_PARTS // 2)
    def _(i):
        wq_copy(i).start()
        first_head_copy(k_hbm, k_buf, k_sem, i).start()

    @pl.loop(0, WQ_PARTS // 2)
    def _(i):
        wq_copy(WQ_PARTS // 2 + i).start()
        first_head_copy(v_hbm, v_buf, v_sem, i).start()

    def gather_copy(g, slot, owner):
        half = SLOT_HALF[slot]
        if g == GATHER_WO:
            rows = WO_SHARE[owner] - WO_SPLIT[owner] if half else WO_SPLIT[owner]
            ref = wo_late.at[pl.ds(WO_START[owner] + half * WO_SPLIT[owner], rows)]
        else:
            ref = (x_all, q_all)[g].at[2 * owner + half]
        i = N_SLOT * g + slot
        return remote(ref, ref, g_send.at[i], g_recv.at[i], 3 if slot % 2 else 1)

    def each_gather_copy(g, slots, offsets, action):
        for slot in slots:
            if g == GATHER_WO:
                for owner in WO_OWNERS:
                    on_chip(owner - offsets[slot])(
                        lambda slot=slot, owner=owner: action(gather_copy(g, slot, owner)))
            else:
                action(gather_copy(g, slot, ahead(offsets[slot])))

    def send(g, slots):
        each_gather_copy(g, slots, OWNER_FROM_SENDER, lambda copy: copy.start())

    def receive(g, slots):
        each_gather_copy(g, slots, OWNER_FROM_RECEIVER, lambda copy: copy.wait_recv())

    def relay(g):
        for slot in (0, 1):
            receive(g, (slot,))
            send(g, (slot + 4,))

    acc[...] = jnp.zeros_like(acc)
    x_copy.wait()
    x_all[pl.ds(2 * me, 2)] = x_mine[...].astype(BF16).reshape(2, QB // 2, DM)
    pl.semaphore_wait(barrier, N_DEV - 1)
    send(GATHER_X, (0, 1, 2, 3))
    relay(GATHER_X)
    for h in range(1, EARLY_HEADS):
        for copy in head_copies(h):
            copy.start()

    for c in WO_OWNERS:
        @on_chip(c)
        def _(c=c):
            wo_mine_copy(c).wait()
            wo_late[pl.ds(WO_START[c], WO_SHARE[c])] = (
                wo_mine[pl.ds(0, WO_SHARE[c])].astype(BF16))

    send(GATHER_WO, (0, 1))
    wait_filled(wq_mine, w_sem.at[1])
    receive(GATHER_X, (2, 3, 4, 5))
    q = jnp.dot(x_all[...].reshape(SQ, DM), wq_mine[...].astype(BF16),
                preferred_element_type=F32) * Q_SCALE
    for i in (0, 1):
        q_all[2 * me + i] = q[:, i * DH:(i + 1) * DH].astype(BF16).reshape(NQB, QB, DH)
    send(GATHER_Q, (0, 1, 2, 3))
    relay(GATHER_Q)
    send(GATHER_WO, (2, 3))
    relay(GATHER_WO)
    receive(GATHER_Q, (2, 3, 4, 5))

    row = lax.broadcasted_iota(jnp.int32, (QB, DH), 0)
    lane = lax.broadcasted_iota(jnp.int32, (QB, DH), 1)
    on_diagonal = (lane & (QB - 1)) == row

    hops = []
    for i in range(N_DEV - 1):
        d = jnp.int32(HOP_ORDER[0][i])
        for c in range(1, N_DEV):
            d = jnp.where(me == c, HOP_ORDER[c][i], d)
        hops.append(d)

    def send_stat(n, d):
        remote(stat.at[n, 0], stat.at[n, d], s_send, s_recv.at[n], d).start()

    def send_part(n, d):
        remote(part.at[n, 0], part.at[n, d], p_send, p_recv.at[n], d).start()

    def wait_stats(n):
        wait_filled(stat.at[n, pl.ds(1, N_DEV - 1)], s_recv.at[n])

    def wait_parts(n):
        wait_filled(part.at[n, pl.ds(1, N_DEV - 1)], p_recv.at[n])

    def probabilities(n):
        k = k_buf[n >> 2, :, n & 3].reshape(NKB * QB, DH).astype(BF16)
        s = lax.dot_general(q_all[n >> 2, n & 3], k, (((1,), (1,)), ((), ())),
                            preferred_element_type=F32)
        row_max = jnp.max(s, axis=1, keepdims=True)
        p = jnp.exp2(s - row_max)
        p_buf[...] = p.astype(BF16)
        lane_sums = p[:, :DH]
        for i in range(1, NKB * QB // DH):
            lane_sums = lane_sums + p[:, i * DH:(i + 1) * DH]
        return row_max, lane_sums

    def store_stats(n, row_max, lane_sums):
        for i, column in enumerate((row_max, jnp.sum(lane_sums, axis=1, keepdims=True))):
            stat[n, 0, pl.ds(i, 1)] = jnp.sum(
                jnp.where(on_diagonal, column, 0.0), axis=0, keepdims=True)

    def weighted_values(n, start=0, size=NKB):
        v = v_buf[n >> 2, pl.ds(start, size), n & 3].reshape(size * QB, DH).astype(BF16)
        return jnp.dot(p_buf[:, pl.ds(start * QB, size * QB)], v, preferred_element_type=F32)

    def merge_weights(n):
        m = [stat[n, d, pl.ds(0, 1)] for d in range(N_DEV)]
        top = jnp.maximum(jnp.maximum(m[0], m[1]), jnp.maximum(m[2], m[3]))
        e = [jnp.exp2(local - top) for local in m]
        inv = 1.0 / sum(e[d] * stat[n, d, pl.ds(1, 1)] for d in range(N_DEV))
        for a in (0, 1):
            pair = jnp.where(lane[:1] < QB, e[2 * a], e[2 * a + 1]) * inv
            w_buf[n & 1, pl.ds(a * DH, DH)] = jnp.broadcast_to(pair, (DH, DH)).T

    def merged(n):
        t = [w_buf[n & 1, pl.ds(d * QB, QB)] * part[n, d].astype(F32) for d in range(N_DEV)]
        return ((t[0] + t[1]) + (t[2] + t[3])).astype(BF16)

    pl.loop(N_EARLY, NPIECE - NQB)(fetch)

    @pl.loop(0, N_EARLY)
    def _(n):
        @pl.when((n & 3) == 0)
        def _():
            wait_filled(k_buf.at[n >> 2], k_sem.at[n])
            wait_filled(v_buf.at[n >> 2], v_sem.at[n])

        store_stats(n, *probabilities(n))
        part[n, 0] = weighted_values(n).astype(BF16)
        to_owner = (n + N_DEV - me) & (N_DEV - 1)

        @pl.when(to_owner != 0)
        def _():
            send_stat(n, to_owner)
            send_part(n, to_owner)

    def late_piece(n, weights_for=None):
        k_copy(n).wait()
        store_stats(n, *probabilities(n))
        for d in hops:
            send_stat(n, d)
        if weights_for is not None:
            wait_stats(weights_for)
        v_copy(n).wait()
        if weights_for is not None:
            merge_weights(weights_for)
        part[n, 0] = weighted_values(n).astype(BF16)
        for d in hops:
            send_part(n, d)

    pl.loop(N_EARLY, N_EARLY + LAG)(late_piece)

    @pl.loop(0, EARLY_HEADS)
    def _(h):
        n = h * NQB + me
        wait_stats(n)
        wait_parts(n)
        merge_weights(n)
        ctx[me, h] = merged(n)

    def ctx_copy(d, owner):
        return remote(ctx.at[owner], ctx.at[owner], c_send.at[d - 1], c_recv.at[d - 1], d)

    for d in (2, 1, 3):
        ctx_copy(d, me).start()
    receive(GATHER_WO, (2, 3, 4, 5))

    @pl.loop(N_EARLY + LAG, LAST)
    def _(n):
        @pl.when(n == NPIECE - 2 * NQB)
        def _():
            pl.loop(NPIECE - NQB, LAST)(fetch)
            k_copy(LAST).start()
            last_v_copy(0).start()
            last_v_copy(1).start()
            pl.when(me != 2)(fetch_wo_early)

        done = n - LAG
        late_piece(n, done)
        wait_parts(done)
        wo = wo_late[pl.ds(pl.multiple_of(((done >> 2) - EARLY_HEADS) * DH, DH), DH)]
        rows = pl.ds(pl.multiple_of((done & 3) * QB, QB), QB)
        acc[rows] += jnp.dot(merged(done), wo, preferred_element_type=F32)

    for d in range(1, N_DEV):
        ctx_copy(d, ahead(N_DEV - d)).wait_recv()
        ctx_copy(d, me).wait_send()
    for g in (GATHER_X, GATHER_Q, GATHER_WO):
        each_gather_copy(g, range(N_SLOT), OWNER_FROM_SENDER, lambda copy: copy.wait_send())

    k_copy(LAST).wait()
    row_max, lane_sums = probabilities(LAST)
    carry[0] = jnp.broadcast_to(row_max, (QB, DH))
    carry[1] = lane_sums
    last_v_copy(0).wait()
    carry[2] = weighted_values(LAST, 0, NKB // 2)
    store_stats(LAST, carry[0], carry[1])
    for d in hops:
        send_stat(LAST, d)
    last_v_copy(1).wait()
    local = carry[2] + weighted_values(LAST, NKB // 2, NKB // 2)
    for start, size in ((0, LEAD_ROWS), (LEAD_ROWS, QB - LEAD_ROWS)):
        rows = pl.ds(start, size)
        part[LAST, 0, rows] = local[start:start + size].astype(BF16)
        remote(part.at[LAST, 0, rows], part.at[LAST, hops[0], rows],
               p_send, p_recv.at[LAST], hops[0]).start()
    for d in hops[1:]:
        send_part(LAST, d)
    on_chip(2)(fetch_wo_early)

    def finish(steps):
        for i, (chunk, piece, weights_for) in enumerate(steps):
            if i == len(steps) - 1:
                sent = (pl.ds(0, EARLY_HEADS + NPIECE - N_EARLY), pl.ds(1, N_DEV - 1))
                wait_filled(stat.at[sent], s_send)
                wait_filled(part.at[sent], p_send)
            if chunk is not None:
                wo_early_copy(chunk).wait()
            if piece is not None:
                wait_parts(piece)
            if weights_for is not None:
                wait_stats(weights_for)

            if chunk is not None:
                h, c = divmod(chunk, COL_PARTS)
                cols = pl.ds(c * WO_COLS, WO_COLS)
                total = acc[:, cols] + jnp.dot(
                    ctx[:, h].reshape(SQ, DH), wo_early[chunk].astype(BF16),
                    preferred_element_type=F32)
                acc[:, cols] = total
                if h == EARLY_HEADS - 1:
                    out_ref[:, cols] = total.astype(out_ref.dtype)
            if piece is not None:
                h, j = divmod(piece, NQB)
                rows = pl.ds(j * QB, QB)
                total = acc[rows] + jnp.dot(
                    merged(piece), wo_late[pl.ds((h - EARLY_HEADS) * DH, DH)],
                    preferred_element_type=F32)
                if chunk is None:
                    out_ref[rows] = total.astype(out_ref.dtype)
                else:
                    acc[rows] = total
            if weights_for is not None:
                merge_weights(weights_for)

    pl.when(me == 3)(lambda: finish(FINISH_CHIP_3))
    pl.when(me != 3)(lambda: finish(FINISH))


def pallas_dist_sparse_attn_strided_kvseq_b1_sq256_skv4096_hq8_dh128_kernel(
    x: jax.Array,
    Wq: jax.Array,
    K_ext: jax.Array,
    V_ext: jax.Array,
    Wo: jax.Array,
):
    dma = pltpu.SemaphoreType.DMA
    kv_shape = (NKB, NQB, QB, HQ, DH)
    out = pl.pallas_call(
        _body,
        out_shape=jax.ShapeDtypeStruct((SQ, DM), BF16),
        in_specs=[pl.BlockSpec(memory_space=pl.ANY)] * 5,
        out_specs=pl.BlockSpec(memory_space=pltpu.VMEM),
        scratch_shapes=[
            pltpu.VMEM((QB, DM), F32),
            pltpu.VMEM((DM, 2 * DH), F32),
            pltpu.VMEM((max(WO_SHARE), DM), F32),
            pltpu.VMEM((N_CHUNK, DH, WO_COLS), F32),
            pltpu.VMEM((HQ, NKB, NQB, QB, DH), F32),
            pltpu.VMEM((HQ, NKB, NQB, QB, DH), F32),
            pltpu.VMEM((2 * N_DEV, QB // 2, DM), BF16),
            pltpu.VMEM((HQ, NQB, QB, DH), BF16),
            pltpu.VMEM((DM - EARLY_HEADS * DH, DM), BF16),
            pltpu.VMEM((QB, NKB * QB), BF16),
            pltpu.VMEM((3, QB, DH), F32),
            pltpu.VMEM((2, N_DEV * QB, DH), F32),
            pltpu.VMEM((NPIECE, N_DEV, QB, DH), BF16),
            pltpu.VMEM((NPIECE, N_DEV, 2, DH), F32),
            pltpu.VMEM((NQB, EARLY_HEADS, QB, DH), BF16),
            pltpu.VMEM((SQ, DM), F32),
            dma((3,)), dma((NPIECE,)), dma((NPIECE + 1,)), dma((N_CHUNK,)),
            dma((3 * N_SLOT,)), dma((3 * N_SLOT,)), dma((N_DEV - 1,)), dma((N_DEV - 1,)),
            dma, dma, dma((NPIECE,)), dma((NPIECE,)),
        ],
        compiler_params=pltpu.CompilerParams(
            collective_id=0,
            vmem_limit_bytes=64 << 20,
            disable_bounds_checks=True,
            disable_semaphore_checks=True,
        ),
    )(x.reshape(SQ, DM), Wq, K_ext.reshape(kv_shape), V_ext.reshape(kv_shape), Wo)
    return out.reshape(1, SQ, DM)
```
